```python
import numpy as np

kernel_name = "dist_mlpseq_tp2d_cs_cs_b64_d2048_h4096"

def setup_inputs():
    x = np.random.randn(64, 4096).astype(np.float32)
    Win0 = np.random.randn(4096, 8192).astype(np.float32)
    Wout0 = np.random.randn(8192, 4096).astype(np.float32)
    Win1 = np.random.randn(4096, 8192).astype(np.float32)
    Wout1 = np.random.randn(8192, 4096).astype(np.float32)
    Win2 = np.random.randn(4096, 8192).astype(np.float32)
    Wout2 = np.random.randn(8192, 4096).astype(np.float32)
    return {"x": x, "Win0": Win0, "Wout0": Wout0, "Win1": Win1, "Wout1": Wout1, "Win2": Win2, "Wout2": Wout2}

def reference(x, Win0, Win1, Win2, Wout0, Wout1, Wout2):
    h = x @ Win0
    h = np.maximum(h, 0.0)
    x = h @ Wout0
    h = x @ Win1
    h = np.maximum(h, 0.0)
    x = h @ Wout1
    h = x @ Win2
    h = np.maximum(h, 0.0)
    x = h @ Wout2
    return x
```

```python
import jax
import jax.numpy as jnp
from jax import lax
from jax.experimental import pallas as pl
from jax.experimental.pallas import tpu as pltpu

F32, BF16 = jnp.float32, jnp.bfloat16
B, D, H = 64, 2048, 4096
NS = 16
RA, RB = 64, 128


def build(q0=3, xfwd=True, nosemcheck=True, nobounds=True, lastk=(2048, 1024, 512, 512), scopes=False,
          last_rows=128, last_q0=3, tail="full", flags=None):
    MESH = pl.DeviceIdType.MESH
    groups = (8, 4, 2, 1, 1)
    scope = jax.named_scope if scopes else (lambda n: _Null())

    def body(x_hbm, a0, b0, a1, b1, a2, b2, out,
             wa, wb, xf, xb, hacc, hb, oacc, hsend, hrecv, osend, orecv,
             wsem, gsem, lsem, xsem, hs_sem, hr_sem, os_sem, or_sem, fs_sem, fr_sem, xs_sem, xr_sem):
        mx, my = lax.axis_index("x"), lax.axis_index("y")
        xn, yn = (1 - mx, my), (mx, 1 - my)
        wins, wouts = (a0, a1, a2), (b0, b1, b2)

        def lanes(c):
            return pl.ds(c * 128, 128) if isinstance(c, int) else pl.ds(pl.multiple_of(c * 128, 128), 128)

        def rows8(u):
            return pl.ds(u * 8, 8) if isinstance(u, int) else pl.ds(pl.multiple_of(u * 8, 8), 8)

        def issue(w_hbm, buf, m, u, c, sem):
            for s0, n, p in ((0, q0, 0), (q0, NS - q0, 1)):
                src = w_hbm.at[pl.ds(m * NS + s0, n), rows8(u), lanes(c)]
                dst = buf.at[c, pl.ds(m * NS + s0, n), rows8(u), :]
                pltpu.make_async_copy(src, dst, sem).start(priority=p)

        def wtile(buf, c, s0, n):
            v = buf[c, pl.ds(s0, n)]
            return v.reshape(v.shape[0] * v.shape[1], 128).astype(BF16)

        def wait_ref(v, sem):
            pltpu.make_async_copy(v, v, sem).wait()

        def wait_mb(buf, m, sem):
            wait_ref(buf.at[:, pl.ds(m * NS, NS)], sem)

        def issue_unit(w, m, i):
            k = w // 2
            if w % 2 == 0:
                for j in range(8):
                    issue(wins[k], wa, m, i // 4, (i % 4) * 8 + j, wsem.at[m])
            else:
                for j in range(8):
                    issue(wouts[k], wb, m, i // 2, (i % 2) * 8 + j, wsem.at[2 + m])

        def issue_group_unit(g, i, m=None):
            c0, n = sum(groups[:g]), groups[g]
            for j in range(8):
                if n >= 8:
                    t = i // (n // 8)
                    c = c0 + (i % (n // 8)) * 8 + j
                else:
                    t = i * (8 // n) + j // n
                    c = c0 + j % n
                if m is None:
                    issue(b2, wb, t // 16, t % 16, c, gsem.at[g])
                else:
                    issue(b2, wb, m, t, c, gsem.at[g])

        def up(k, m, c):
            r = jnp.dot(xb[:, m * 1024:(m + 1) * 1024], wtile(wa, c, m * NS, NS), preferred_element_type=F32)
            if m == 0:
                hacc[c] = r
            else:
                r = hacc[c] + r
                hacc[c] = r
                hsend[k, c] = r.astype(BF16)

        def down(k, m, c):
            r = jnp.dot(hb[:, m * 2048:(m + 1) * 2048], wtile(wb, c, m * NS, NS), preferred_element_type=F32)
            if m == 0:
                oacc[c] = r
            else:
                r = oacc[c] + r
                oacc[c] = r
                osend[k, c] = r.astype(BF16)

        def h_copy(k, half):
            return pltpu.make_async_remote_copy(
                hsend.at[k, pl.ds(half * 16, 16)], hrecv.at[k, pl.ds(half * 16, 16)],
                hs_sem, hr_sem.at[2 * k + half], device_id=yn, device_id_type=MESH)

        def o_copy(k, half):
            return pltpu.make_async_remote_copy(
                osend.at[k, pl.ds(half * 8, 8)], orecv.at[k, pl.ds(half * 8, 8)],
                os_sem, or_sem.at[2 * k + half], device_id=xn, device_id_type=MESH)

        def g_copy(g):
            c0, n = sum(groups[:g]), groups[g]
            return pltpu.make_async_remote_copy(
                osend.at[2, pl.ds(c0, n)], orecv.at[2, pl.ds(c0, n)],
                fs_sem, fr_sem.at[g], device_id=xn, device_id_type=MESH)

        def h_finish(k, half):
            h_copy(k, half).wait_recv()
            for c in range(half * 16, half * 16 + 16):
                v = hacc[c] + hrecv[k, c].astype(F32)
                hb[:, c * 128:(c + 1) * 128] = jnp.maximum(v, 0.0).astype(BF16)

        def o_finish(k, half):
            o_copy(k, half).wait_recv()
            for c in range(half * 8, half * 8 + 8):
                v = oacc[c] + orecv[k, c].astype(F32)
                xb[:, c * 128:(c + 1) * 128] = v.astype(BF16)

        def seg(n, *fs):
            @pl.loop(0, n)
            def _(i):
                for f in fs:
                    f(i)

        x_copy = lambda: pltpu.make_async_copy(x_hbm, xf, xsem)
        x_send = lambda: pltpu.make_async_remote_copy(xb, xb, xs_sem, xr_sem, device_id=xn, device_id_type=MESH)
        issue_unit(0, 0, 0)
        if xfwd:
            pl.when(mx == 0)(lambda: x_copy().start())
        else:
            x_copy().start()
        bar = pltpu.get_barrier_semaphore()
        for nb in (xn, yn):
            pl.semaphore_signal(bar, inc=1, device_id=nb, device_id_type=MESH)
        seg(23, lambda i: issue_unit(0, 0, i + 1))
        pl.semaphore_wait(bar, 2)
        if xfwd:
            @pl.when(mx == 0)
            def _():
                x_copy().wait()
                xb[...] = xf[...].astype(BF16)
                x_send().start()
        else:
            x_copy().wait()
            xb[...] = xf[...].astype(BF16)
        seg(8, lambda i: issue_unit(0, 0, i + 24))
        for k in range(3):
            w = 2 * k
            if k == 0:
                seg(16, lambda i: issue_unit(w, 1, i))
                if xfwd:
                    pl.when(mx == 0)(lambda: x_send().wait_send())
                    pl.when(mx == 1)(lambda: x_send().wait_recv())
            else:
                seg(8, lambda i: issue_unit(w, 1, 2 * i), lambda i: issue_unit(w, 1, 2 * i + 1), lambda i: down(k - 1, 1, 8 + i))
                o_copy(k - 1, 1).start()
                o_finish(k - 1, 0)
            wait_mb(wa, 0, wsem.at[0])
            seg(16, lambda i: issue_unit(w, 1, 16 + i), lambda i: up(k, 0, i))
            if k < 2:
                seg(16, lambda i: issue_unit(w + 1, 0, i), lambda i: up(k, 0, 16 + i))
                if k > 0:
                    o_finish(k - 1, 1)
                wait_mb(wa, 1, wsem.at[1])
                seg(16, lambda i: issue_unit(w + 1, 0, 16 + i), lambda i: up(k, 1, i))
                h_copy(k, 0).start()
                seg(16, lambda i: issue_unit(w + 1, 1, i), lambda i: up(k, 1, 16 + i))
                h_copy(k, 1).start()
                h_finish(k, 0)
                wait_mb(wb, 0, wsem.at[2])
                seg(8, lambda i: issue_unit(w + 1, 1, 16 + 2 * i), lambda i: issue_unit(w + 1, 1, 17 + 2 * i), lambda i: down(k, 0, i))
                seg(8, lambda i: issue_unit(w + 2, 0, 2 * i), lambda i: issue_unit(w + 2, 0, 2 * i + 1), lambda i: down(k, 0, 8 + i))
                h_finish(k, 1)
                wait_mb(wb, 1, wsem.at[3])
                seg(8, lambda i: issue_unit(w + 2, 0, 16 + 2 * i), lambda i: issue_unit(w + 2, 0, 17 + 2 * i), lambda i: down(k, 1, i))
                o_copy(k, 0).start()

        def fin(g):
            c0, n = sum(groups[:g]), groups[g]
            g_copy(g).wait_recv()
            for c in range(c0, c0 + n):
                out[:, c * 128:(c + 1) * 128] = oacc[c] + orecv[2, c].astype(F32)

        def issue_last(rows):
            s = 32 - rows // 128
            for i, kk in enumerate(lastk):
                for _ in range(kk // 128):
                    for r0, n, p in ((0, 8 * last_q0, 0), (8 * last_q0, 128 - 8 * last_q0, 1)):
                        if n:
                            pltpu.make_async_copy(b2.at[s, pl.ds(r0, n), lanes(15)], wb.at[15, s, pl.ds(r0, n), :],
                                                  lsem.at[i]).start(priority=p)
                    s += 1
            assert s == 32

        def sends_done():
            wait_ref(hsend, hs_sem)
            wait_ref(osend.at[pl.ds(0, 2)], os_sem)

        if tail == "full":
            gi = issue_group_unit
            seg(8, lambda i: gi(0, i), lambda i: up(2, 0, 16 + 2 * i), lambda i: up(2, 0, 17 + 2 * i))
            seg(4, lambda i: gi(0, 8 + i))
            o_finish(1, 1)
            wait_mb(wa, 1, wsem.at[1])
            seg(8, lambda i: gi(0, 12 + i), lambda i: up(2, 1, 2 * i), lambda i: up(2, 1, 2 * i + 1))
            h_copy(2, 0).start()
            seg(8, lambda i: gi(0, 20 + i), lambda i: up(2, 1, 16 + 2 * i), lambda i: up(2, 1, 17 + 2 * i))
            h_copy(2, 1).start()
            seg(4, lambda i: gi(0, 28 + i))
            seg(12, lambda i: gi(1, i))
            h_finish(2, 0)
            h_finish(2, 1)
            wait_ref(wb.at[pl.ds(0, 8)], gsem.at[0])
            seg(4, lambda i: gi(1, 12 + i), lambda i: down(2, 0, i), lambda i: down(2, 1, i))
            seg(4, lambda i: gi(2, i), lambda i: down(2, 0, 4 + i), lambda i: down(2, 1, 4 + i))
            g_copy(0).start()
            seg(4, lambda i: gi(2, 4 + i))
            wait_ref(wb.at[pl.ds(8, 4)], gsem.at[1])
            seg(4, lambda i: gi(3, i), lambda i: down(2, 0, 8 + i), lambda i: down(2, 1, 8 + i))
            g_copy(1).start()
            issue_last(4096)
            sends_done()
            fin(0)
            for g in (2, 3):
                c0, n = sum(groups[:g]), groups[g]
                with scope(f"w_g{g}"):
                    wait_ref(wb.at[pl.ds(c0, n)], gsem.at[g])
                with scope(f"c_g{g}"):
                    seg(n, lambda i: down(2, 0, c0 + i), lambda i: down(2, 1, c0 + i))
                    g_copy(g).start()
                with scope(f"f_g{g-1}"):
                    fin(g - 1)
            s, acc = 0, None
        else:
            gi = lambda g, i: issue_group_unit(g, i, 1)
            seg(8, lambda i: issue_unit(5, 0, i), lambda i: up(2, 0, 16 + 2 * i), lambda i: up(2, 0, 17 + 2 * i))
            seg(4, lambda i: issue_unit(5, 0, 8 + i))
            o_finish(1, 1)
            wait_mb(wa, 1, wsem.at[1])
            seg(8, lambda i: issue_unit(5, 0, 12 + i), lambda i: up(2, 1, 2 * i), lambda i: up(2, 1, 2 * i + 1))
            h_copy(2, 0).start()
            seg(8, lambda i: issue_unit(5, 0, 20 + i), lambda i: up(2, 1, 16 + 2 * i), lambda i: up(2, 1, 17 + 2 * i))
            h_copy(2, 1).start()
            seg(4, lambda i: issue_unit(5, 0, 28 + i))
            seg(10, lambda i: gi(0, i))
            h_finish(2, 0)
            wait_mb(wb, 0, wsem.at[2])
            seg(6, lambda i: gi(0, 10 + i), lambda i: down(2, 0, i))
            h_finish(2, 1)
            seg(5, lambda i: gi(1, i), lambda i: down(2, 0, 6 + 2 * i), lambda i: down(2, 0, 7 + 2 * i))
            seg(3, lambda i: gi(1, 5 + i))
            with scope(f"w_g0"):
                wait_ref(wb.at[pl.ds(0, 8), pl.ds(16, 16)], gsem.at[0])
            seg(4, lambda i: gi(2, i), lambda i: down(2, 1, 2 * i), lambda i: down(2, 1, 2 * i + 1))
            g_copy(0).start()
            seg(2, lambda i: gi(3, i))
            issue_last(2048)
            sends_done()
            for g in (1, 2, 3):
                c0, n = sum(groups[:g]), groups[g]
                with scope(f"w_g{g}"):
                    wait_ref(wb.at[pl.ds(c0, n), pl.ds(16, 16)], gsem.at[g])
                with scope(f"c_g{g}"):
                    seg(n, lambda i: down(2, 1, c0 + i))
                    g_copy(g).start()
                if g > 1:
                    with scope(f"f_g{g-2}"):
                        fin(g - 2)
            s, acc = 16, oacc[15]
        for i, kk in enumerate(lastk):
            n = kk // 128
            with scope(f"w_l{i}"):
                wait_ref(wb.at[15, pl.ds(s, n)], lsem.at[i])
            with scope(f"c_l{i}"):
                r = jnp.dot(hb[:, s * 128:(s + n) * 128], wtile(wb, 15, s, n), preferred_element_type=F32)
                acc = r if acc is None else acc + r
            s += n
        with scope("send"):
            osend[2, 15] = acc.astype(BF16)
            g_copy(4).start()
            oacc[15] = acc
        with scope("f_g3"):
            if tail != "full":
                fin(2)
            fin(3)
        with scope("f_g4"):
            fin(4)
        with scope("s_done"):
            wait_ref(osend.at[2], fs_sem)

    def fn(x, Win0, Wout0, Win1, Wout1, Win2, Wout2):
        ra = lambda a: a.reshape(D // RA, RA, H)
        rb = lambda a: a.reshape(H // RB, RB, D)
        DMA = pltpu.SemaphoreType.DMA
        return pl.pallas_call(
            body,
            out_shape=jax.ShapeDtypeStruct((B, D), F32),
            in_specs=[pl.BlockSpec(memory_space=pltpu.HBM)] * 7,
            out_specs=pl.BlockSpec(memory_space=pltpu.VMEM),
            scratch_shapes=[
                pltpu.VMEM((32, 32, RA, 128), F32), pltpu.VMEM((16, 32, RB, 128), F32),
                pltpu.VMEM((B, D), F32), pltpu.VMEM((B, D), BF16),
                pltpu.VMEM((32, B, 128), F32), pltpu.VMEM((B, H), BF16), pltpu.VMEM((16, B, 128), F32),
                pltpu.VMEM((3, 32, B, 128), BF16), pltpu.VMEM((3, 32, B, 128), BF16),
                pltpu.VMEM((3, 16, B, 128), BF16), pltpu.VMEM((3, 16, B, 128), BF16),
                DMA((4,)), DMA((4,)), DMA((len(lastk),)), DMA, DMA, DMA((6,)), DMA, DMA((4,)),
                DMA, DMA((5,)), DMA, DMA,
            ],
            compiler_params=pltpu.CompilerParams(
                vmem_limit_bytes=100 * 2**20, collective_id=0, flags=flags,
                disable_bounds_checks=nobounds, disable_semaphore_checks=nosemcheck),
        )(x, ra(Win0), rb(Wout0), ra(Win1), rb(Wout1), ra(Win2), rb(Wout2))
    return fn


class _Null:
    def __enter__(self):
        return self

    def __exit__(self, *a):
        return False


def pallas_dist_mlpseq_tp2d_cs_cs_b64_d2048_h4096_kernel(x, Win0, Wout0, Win1, Wout1, Win2, Wout2):
    return build(tail="half", lastk=(1024, 512, 512), q0=2)(x, Win0, Wout0, Win1, Wout1, Win2, Wout2)
```

```python
import jax
import jax.numpy as jnp
from jax import lax
from jax.experimental import pallas as pl
from jax.experimental.pallas import tpu as pltpu

F32, BF16 = jnp.float32, jnp.bfloat16
B, D, H = 64, 2048, 4096
LANES = 128
D_STRIPS, H_STRIPS = D // LANES, H // LANES
LAYERS = 3

STREAMS = 16
IN_ROWS, OUT_ROWS = 64, 128
STEP_SPLIT = ((11, 1), (5, 0))
UNIT = 8
UNITS = 32
BLOCK_LAG, GROUP_LAG = 8, 7

GROUPS = ((0, 8), (8, 4), (12, 2), (14, 1))
LAST_STRIP = D_STRIPS - 1
LAST_PIECES = ((16, 8), (24, 4), (28, 4))
LAST_SPLIT = ((88, 1), (40, 0))
LAST_PARTS, LAST_ROWS = 4, B // 4


def _mlp_body(
    x_hbm, win0, wout0, win1, wout1, win2, wout2, out,
    win, wout, x_f32, xs, h_acc, hs, o_acc, h_send, h_recv, o_send, o_recv,
    block_sem, group_sem, piece_sem, x_sem,
    h_send_sem, h_recv_sem, o_send_sem, o_recv_sem, f_send_sem, f_recv_sem,
):
    mx, my = lax.axis_index("x"), lax.axis_index("y")
    x_peer, y_peer = (1 - mx, my), (mx, 1 - my)
    weights = (win0, wout0, win1, wout1, win2, wout2)
    last_block, last_layer = 4 * LAYERS - 1, LAYERS - 1

    def load_step(w_hbm, w_vmem, half, panel, strip, sem):
        rows = pl.ds(pl.multiple_of(panel * 8, 8), 8)
        cols = pl.ds(pl.multiple_of(strip * LANES, LANES), LANES)
        first = half * STREAMS
        for n, priority in STEP_SPLIT:
            streams = pl.ds(first, n)
            pltpu.make_async_copy(
                w_hbm.at[streams, rows, cols], w_vmem.at[strip, streams, rows, :], sem
            ).start(priority=priority)
            first += n

    def load_units(w_hbm, w_vmem, half, strip0, strips, sem, lo, hi, work):
        shift = strips.bit_length() - 1

        @pl.loop(lo, hi)
        def _(unit):
            for j in range(UNIT):
                step = unit * UNIT + j
                load_step(w_hbm, w_vmem, half, step >> shift, strip0 + (step & (strips - 1)), sem)
            work(unit)

    def stream(block, lo, hi, work=lambda i: None):
        w, half = divmod(block, 2)
        if block < last_block:
            w_vmem, strips = (wout, D_STRIPS) if w % 2 else (win, H_STRIPS)
            load_units(weights[w], w_vmem, half, 0, strips, block_sem.at[block % 4],
                       lo, hi, lambda unit: work(unit - lo))
            return
        for g, (strip0, strips) in enumerate(GROUPS):
            base = 2 * strip0
            a, b = max(lo, base), min(hi, base + 2 * strips)
            if a < b:
                load_units(wout2, wout, 1, strip0, strips, group_sem.at[g],
                           a - base, b - base, lambda unit: work(unit + base - lo))

    def load_last_strip():
        cols = pl.ds(LAST_STRIP * LANES, LANES)
        for i, (first, n) in enumerate(LAST_PIECES):
            for s in range(first, first + n):
                row = 0
                for count, priority in LAST_SPLIT:
                    rows = pl.ds(row, count)
                    pltpu.make_async_copy(
                        wout2.at[s, rows, cols], wout.at[LAST_STRIP, s, rows, :], piece_sem.at[i]
                    ).start(priority=priority)
                    row += count

    def wait_filled(region, sem):
        pltpu.make_async_copy(region, region, sem).wait()

    def matmul(act, strip0, w):
        k = w.shape[0] * w.shape[1]
        lhs = jnp.concatenate([act[strip0 + i] for i in range(k // LANES)], axis=1)
        return jnp.dot(lhs, w.reshape(k, LANES).astype(BF16), preferred_element_type=F32)

    def accumulate(act, w_vmem, acc, send, layer, half, strip):
        r = matmul(act, half * act.shape[0] // 2, w_vmem[strip, pl.ds(half * STREAMS, STREAMS)])
        if half:
            r = acc[strip] + r
            send[layer, strip] = r.astype(BF16)
        acc[strip] = r

    def up(layer, half, strip):
        accumulate(xs, win, h_acc, h_send, layer, half, strip)

    def down(layer, half, strip):
        accumulate(hs, wout, o_acc, o_send, layer, half, strip)

    def remote(src, dst, send_sem, recv_sem, peer):
        return pltpu.make_async_remote_copy(
            src, dst, send_sem, recv_sem, device_id=peer, device_id_type=pl.DeviceIdType.MESH
        )

    def h_copy(layer, half):
        at, i = (layer, pl.ds(half * H_STRIPS // 2, H_STRIPS // 2)), 2 * layer + half
        return remote(h_send.at[at], h_recv.at[at], h_send_sem.at[i], h_recv_sem.at[i], y_peer)

    def o_copy(layer, half):
        at, i = (layer, pl.ds(half * D_STRIPS // 2, D_STRIPS // 2)), 2 * layer + half
        return remote(o_send.at[at], o_recv.at[at], o_send_sem.at[i], o_recv_sem.at[i], x_peer)

    def group_copy(g):
        at = (last_layer, pl.ds(*GROUPS[g]))
        return remote(o_send.at[at], o_recv.at[at], f_send_sem.at[g], f_recv_sem.at[g], x_peer)

    def part_copy(p):
        at, i = (last_layer, LAST_STRIP, pl.ds(p * LAST_ROWS, LAST_ROWS)), len(GROUPS) + p
        return remote(o_send.at[at], o_recv.at[at], f_send_sem.at[i], f_recv_sem.at[i], x_peer)

    def finish_h(layer, half):
        h_copy(layer, half).wait_recv()

        @pl.loop(half * H_STRIPS // 2, (half + 1) * H_STRIPS // 2)
        def _(strip):
            h = h_acc[strip] + h_recv[layer, strip].astype(F32)
            hs[strip] = jnp.maximum(h, 0.0).astype(BF16)

    def finish_o(layer, half):
        o_copy(layer, half).wait_recv()

        @pl.loop(half * D_STRIPS // 2, (half + 1) * D_STRIPS // 2)
        def _(strip):
            xs[strip] = (o_acc[strip] + o_recv[layer, strip].astype(F32)).astype(BF16)

    def x_load():
        return pltpu.make_async_copy(x_hbm, x_f32, x_sem.at[0])

    def x_copy():
        return remote(xs, xs, x_sem.at[1], x_sem.at[2], x_peer)

    stream(0, 0, 1)
    pl.when(mx == 0)(lambda: x_load().start())
    barrier = pltpu.get_barrier_semaphore()
    for peer in (x_peer, y_peer):
        pl.semaphore_signal(barrier, inc=1, device_id=peer, device_id_type=pl.DeviceIdType.MESH)
    stream(0, 1, 20)
    pl.semaphore_wait(barrier, 2)

    @pl.when(mx == 0)
    def _():
        x_load().wait()
        for strip in range(D_STRIPS):
            xs[strip] = x_f32[:, strip * LANES:(strip + 1) * LANES].astype(BF16)
        x_copy().start()

    stream(0, 20, UNITS)

    for block in range(1, last_block + 1):
        prev = block - 1
        layer, is_down, half = prev // 4, prev // 2 % 2, prev % 2
        stream(block, 0, BLOCK_LAG)
        if is_down:
            finish_h(layer, half)
        elif layer > 0:
            finish_o(layer - 1, half)
        elif half == 0:
            pl.when(mx == 0)(lambda: x_copy().wait_send())
            pl.when(mx == 1)(lambda: x_copy().wait_recv())
        w_vmem = wout if is_down else win
        wait_filled(w_vmem.at[:, pl.ds(half * STREAMS, STREAMS)], block_sem.at[prev % 4])
        if block == last_block:
            break
        for part in range(2):
            def work(i):
                if is_down:
                    down(layer, half, 8 * part + i)
                else:
                    up(layer, half, 16 * part + 2 * i)
                    up(layer, half, 16 * part + 2 * i + 1)

            stream(block, BLOCK_LAG + 8 * part, BLOCK_LAG + 8 * part + 8, work)
            if half:
                (o_copy if is_down else h_copy)(layer, part).start()
        stream(block, BLOCK_LAG + 16, UNITS)

    def two_down(half):
        return lambda i: (down(last_layer, half, 2 * i), down(last_layer, half, 2 * i + 1))

    def wait_group(g):
        wait_filled(wout.at[pl.ds(*GROUPS[g]), pl.ds(STREAMS, STREAMS)], group_sem.at[g])

    group0_ready = 16 + GROUP_LAG
    stream(last_block, BLOCK_LAG, BLOCK_LAG + 8, two_down(0))
    finish_h(last_layer, 1)
    stream(last_block, BLOCK_LAG + 8, group0_ready)
    wait_group(0)
    stream(last_block, group0_ready, group0_ready + 4, two_down(1))
    group_copy(0).start()
    stream(last_block, group0_ready + 4, 2 * LAST_STRIP)
    load_last_strip()

    for layer in range(LAYERS):
        for part in range(2):
            h_copy(layer, part).wait_send()
            if layer < last_layer:
                o_copy(layer, part).wait_send()
    for g, (strip0, strips) in enumerate(GROUPS):
        if g > 0:
            wait_group(g)
            pl.loop(strip0, strip0 + strips)(lambda strip: down(last_layer, 1, strip))
            group_copy(g).start()

    acc = o_acc[LAST_STRIP]
    for i, (first, n) in enumerate(LAST_PIECES):
        wait_filled(wout.at[LAST_STRIP, pl.ds(first, n)], piece_sem.at[i])
        acc = acc + matmul(hs, first, wout[LAST_STRIP, pl.ds(first, n)])
    for p in range(LAST_PARTS):
        rows = slice(p * LAST_ROWS, (p + 1) * LAST_ROWS)
        o_send[last_layer, LAST_STRIP, rows] = acc[rows].astype(BF16)
        part_copy(p).start()

    for g, (strip0, strips) in enumerate(GROUPS):
        group_copy(g).wait()
        for strip in range(strip0, strip0 + strips):
            out[:, strip * LANES:(strip + 1) * LANES] = (
                o_acc[strip] + o_recv[last_layer, strip].astype(F32)
            )
    for p in range(LAST_PARTS):
        rows = slice(p * LAST_ROWS, (p + 1) * LAST_ROWS)
        part_copy(p).wait()
        out[rows, LAST_STRIP * LANES:] = (
            acc[rows] + o_recv[last_layer, LAST_STRIP, rows].astype(F32)
        )


def pallas_dist_mlpseq_tp2d_cs_cs_b64_d2048_h4096_kernel(
    x: jax.Array,
    Win0: jax.Array,
    Wout0: jax.Array,
    Win1: jax.Array,
    Wout1: jax.Array,
    Win2: jax.Array,
    Wout2: jax.Array,
):
    def in_streams(w):
        return w.reshape(2 * STREAMS, IN_ROWS, H)

    def out_streams(w):
        return w.reshape(2 * STREAMS, OUT_ROWS, D)

    dma = pltpu.SemaphoreType.DMA
    final_copies = len(GROUPS) + LAST_PARTS
    return pl.pallas_call(
        _mlp_body,
        out_shape=jax.ShapeDtypeStruct((B, D), F32),
        in_specs=[pl.BlockSpec(memory_space=pltpu.HBM)] * 7,
        out_specs=pl.BlockSpec(memory_space=pltpu.VMEM),
        scratch_shapes=[
            pltpu.VMEM((H_STRIPS, 2 * STREAMS, IN_ROWS, LANES), F32),
            pltpu.VMEM((D_STRIPS, 2 * STREAMS, OUT_ROWS, LANES), F32),
            pltpu.VMEM((B, D), F32),
            pltpu.VMEM((D_STRIPS, B, LANES), BF16),
            pltpu.VMEM((H_STRIPS, B, LANES), F32),
            pltpu.VMEM((H_STRIPS, B, LANES), BF16),
            pltpu.VMEM((D_STRIPS, B, LANES), F32),
            pltpu.VMEM((LAYERS, H_STRIPS, B, LANES), BF16),
            pltpu.VMEM((LAYERS, H_STRIPS, B, LANES), BF16),
            pltpu.VMEM((LAYERS, D_STRIPS, B, LANES), BF16),
            pltpu.VMEM((LAYERS, D_STRIPS, B, LANES), BF16),
            dma((4,)),
            dma((len(GROUPS),)),
            dma((len(LAST_PIECES),)),
            dma((3,)),
            dma((2 * LAYERS,)),
            dma((2 * LAYERS,)),
            dma((2 * LAYERS - 2,)),
            dma((2 * LAYERS - 2,)),
            dma((final_copies,)),
            dma((final_copies,)),
        ],
        compiler_params=pltpu.CompilerParams(
            collective_id=0,
            vmem_limit_bytes=100 * 2**20,
            disable_bounds_checks=True,
            disable_semaphore_checks=True,
        ),
    )(
        x,
        in_streams(Win0), out_streams(Wout0),
        in_streams(Win1), out_streams(Wout1),
        in_streams(Win2), out_streams(Wout2),
    )
```
